```python
import numpy as np

kernel_name = "dist_sparse_attn_causalblk_htp_bs_b2_sq256_skv256_hq4_dh64"

def setup_inputs():
    x = np.random.randn(8, 256, 512).astype(np.float32)
    Wq = np.random.randn(512, 1024).astype(np.float32) * 0.02
    K_ext = np.random.randn(8, 256, 16, 64).astype(np.float32)
    V_ext = np.random.randn(8, 256, 16, 64).astype(np.float32)
    Wo = np.random.randn(1024, 512).astype(np.float32) * 0.02
    return {"x": x, "Wq": Wq, "K_ext": K_ext, "V_ext": V_ext, "Wo": Wo}

def reference(x, Wq, K_ext, V_ext, Wo):
    B, Sq, Skv, Hq, Dh = 8, 256, 256, 16, 64
    Q = (x @ Wq).reshape(B, Sq, Hq, Dh)
    qb = (np.arange(Sq) // 64)[:, None]
    kb = (np.arange(Skv) // 64)[None, :]
    mask = kb <= qb
    scores = np.einsum('bihd,bjhd->bhij', Q, K_ext).astype(np.float32) * 0.125
    scores = np.where(mask[None, None, :, :], scores, -1e9)
    scores_max = scores.max(axis=-1, keepdims=True)
    w = np.exp(scores - scores_max)
    row_keep = mask.any(axis=1)
    w_sum = np.where(row_keep[None, None, :, None], w.sum(axis=-1, keepdims=True), 1.0)
    w = w / w_sum
    w = np.where(row_keep[None, None, :, None], w, 0.0)
    ctx = np.einsum('bhij,bjhd->bihd', w, V_ext).reshape(B, Sq, Hq * Dh)
    return ctx @ Wo
```

```python
import functools
import jax
import jax.numpy as jnp
from jax import lax
from jax.experimental import pallas as pl
from jax.experimental.pallas import tpu as pltpu

N_DEV = 4
B_LOC = 2
S = 256
DM = 512
DH = 64
GW = 256
NEG = -1e9
LOG2E = 1.4426950408889634
QSCALE = 0.125 * LOG2E
BF = jnp.bfloat16
F32 = jnp.float32
MESH = pl.DeviceIdType.MESH

NN = (((1,), (0,)), ((), ()))
NT = (((1,), (1,)), ((), ()))


def _dot(a, b, dims=NN):
    return lax.dot_general(a, b, dims, preferred_element_type=F32)


def kernel(x, Wq, K_ext, V_ext, Wo, comm=True, compute=True):
    Kt = jnp.transpose(K_ext, (0, 2, 3, 1)).reshape(8, 16 * DH, S)
    Vt = jnp.transpose(V_ext, (0, 2, 3, 1)).reshape(8, 16 * DH, S)

    def body(x_hbm, wq_hbm, kt_hbm, vt_hbm, wo_hbm, out_ref,
             wq_f, wo_f, x_f, x_b, k_f, v_f, wq_b, wo_b, ctx,
             lsem, ssem, rsem):
        my = lax.axis_index("i")
        right = (my + 1) % N_DEV
        left = (my + 3) % N_DEV

        if comm:
            bar = pltpu.get_barrier_semaphore()
            for nb in (left, right):
                pl.semaphore_signal(bar, inc=1, device_id=(nb,), device_id_type=MESH)

        def lcopy(src, dst, i):
            return pltpu.make_async_copy(src, dst, lsem.at[i])

        ld_wq = [lcopy(wq_hbm.at[:, pl.ds(c * 128, 128)], wq_f.at[c], c) for c in range(2)]
        ld_x = lcopy(x_hbm, x_f, 2)
        ld_wo = lcopy(wo_hbm, wo_f, 3)
        grp = [my, left, right, (my + 2) % N_DEV]

        def kv_copy(src, dst, slot, i):
            rows = pl.ds(pl.multiple_of(grp[slot] * GW, GW), GW)
            return lcopy(src.at[pl.ds(B_LOC * my, B_LOC), rows, :], dst.at[slot], i)

        ld_k = [kv_copy(kt_hbm, k_f, s, 4 + 2 * s) for s in range(4)]
        ld_v = [kv_copy(vt_hbm, v_f, s, 5 + 2 * s) for s in range(4)]

        ld_wq[0].start(); ld_wq[1].start()
        ld_x.start(); ld_k[0].start(); ld_v[0].start(); ld_wo.start()
        for s in range(1, 4):
            ld_k[s].start(); ld_v[s].start()

        def rcopy(src, dst, i, dev):
            return pltpu.make_async_remote_copy(
                src_ref=src, dst_ref=dst, send_sem=ssem.at[i], recv_sem=rsem.at[i],
                device_id=(dev,), device_id_type=MESH)

        cw = [
            rcopy(wq_b.at[0, 0], wq_b.at[1, 0], 0, right),
            rcopy(wq_b.at[0, 1], wq_b.at[1, 1], 1, right),
            rcopy(wq_b.at[1, 0], wq_b.at[3, 0], 2, right),
            rcopy(wo_b.at[0, pl.ds(0, 2)], wo_b.at[1, pl.ds(0, 2)], 3, right),
            rcopy(wo_b.at[0, 2], wo_b.at[1, 2], 4, right),
            rcopy(wo_b.at[1, pl.ds(0, 2)], wo_b.at[3, pl.ds(0, 2)], 5, right),
            rcopy(wo_b.at[0, 3], wo_b.at[1, 3], 6, right),
        ]
        ccw = [
            rcopy(wq_b.at[0, 1], wq_b.at[2, 1], 7, left),
            rcopy(wq_b.at[0, 0], wq_b.at[2, 0], 8, left),
            rcopy(wq_b.at[2, 1], wq_b.at[3, 1], 9, left),
            rcopy(wo_b.at[0, pl.ds(2, 2)], wo_b.at[2, pl.ds(2, 2)], 10, left),
            rcopy(wo_b.at[0, 1], wo_b.at[2, 1], 11, left),
            rcopy(wo_b.at[2, pl.ds(2, 2)], wo_b.at[3, pl.ds(2, 2)], 12, left),
            rcopy(wo_b.at[0, 0], wo_b.at[2, 0], 13, left),
        ]

        def start(k):
            if comm:
                cw[k].start(); ccw[k].start()

        def wait_recv(k):
            if comm:
                cw[k].wait_recv(); ccw[k].wait_recv()

        for c in range(2):
            ld_wq[c].wait()
            wq_b[0, c] = wq_f[c].astype(BF)
        if comm:
            pl.semaphore_wait(bar, 2)
        start(0); start(1)

        ld_x.wait()
        for b in range(B_LOC):
            x_b[b] = x_f[b].astype(BF)

        lane = lax.broadcasted_iota(jnp.int32, (128, 128), 1)
        row = lax.broadcasted_iota(jnp.int32, (128, 128), 0)
        dmask = jnp.logical_and(row < 64, lane >= 64)
        lo_lane = lax.broadcasted_iota(jnp.int32, (S, 128), 1) < 64
        zeros_h = jnp.zeros((DH, S), BF)
        ones_h = jnp.ones((DH, S), BF)
        negc = NEG * LOG2E

        def attn_unit(slot, c, b):
            q = (_dot(x_b[b], wq_b[slot, c]) * QSCALE).astype(BF)
            outs = []
            for hh in range(2):
                r0 = c * 128 + hh * DH
                kt = k_f[slot, b, pl.ds(r0, DH), :].astype(BF)
                vt = v_f[slot, b, pl.ds(r0, DH), :].astype(BF)
                if hh == 0:
                    kz = jnp.concatenate([kt, zeros_h], axis=0)
                    vz = jnp.concatenate([vt, ones_h], axis=0)
                else:
                    kz = jnp.concatenate([zeros_h, kt], axis=0)
                    vz = jnp.concatenate([ones_h, vt], axis=0)
                sa = _dot(q, kz[:, :128])
                sb = _dot(q[128:], kz[:, 128:])
                s_tl = jnp.where(dmask, negc, sa[:128])
                s_bl = sa[128:]
                s_br = jnp.where(dmask, negc, sb)
                m_t = jnp.max(s_tl, axis=1, keepdims=True)
                m_b = jnp.max(jnp.maximum(s_bl, s_br), axis=1, keepdims=True)
                p_tl = jnp.exp2(s_tl - m_t).astype(BF)
                p_bl = jnp.exp2(s_bl - m_b).astype(BF)
                p_br = jnp.exp2(s_br - m_b).astype(BF)
                oa = _dot(jnp.concatenate([p_tl, p_bl], axis=0), vz[:, :128], NT)
                ob = _dot(p_br, vz[:, 128:], NT)
                outs.append(jnp.concatenate([oa[:128], oa[128:] + ob], axis=0))
            num = jnp.where(lo_lane, outs[0], outs[1])
            den = pltpu.roll(jnp.where(lo_lane, outs[1], outs[0]), 64, 1)
            ctx[b, :, pl.ds(slot * GW + c * 128, 128)] = (num / den).astype(BF)

        def attn(slot, c):
            if compute:
                for b in range(B_LOC):
                    attn_unit(slot, c, b)

        def oproj(col, slots, init):
            if not compute:
                return
            for b in range(B_LOC):
                acc = None
                for s in slots:
                    t = _dot(ctx[b, :, pl.ds(s * GW, GW)], wo_b[s, col])
                    acc = t if acc is None else acc + t
                cs = pl.ds(col * 128, 128)
                if init:
                    out_ref[b, :, cs] = acc
                else:
                    out_ref[b, :, cs] += acc

        if not compute:
            out_ref[...] = jnp.zeros(out_ref.shape, F32)

        ld_k[0].wait(); ld_v[0].wait()
        attn(0, 0)
        ld_wo.wait()
        for cc in range(4):
            wo_b[0, cc] = wo_f[:, pl.ds(cc * 128, 128)].astype(BF)
        attn(0, 1)

        wait_recv(0)
        start(2); start(3); start(4)
        ld_k[1].wait(); ld_v[1].wait(); ld_k[2].wait(); ld_v[2].wait()
        attn(1, 0); attn(2, 1)
        wait_recv(1)
        attn(1, 1); attn(2, 0)
        wait_recv(2)
        ld_k[3].wait(); ld_v[3].wait()
        attn(3, 0)
        wait_recv(3)
        start(5); start(6)
        attn(3, 1)
        wait_recv(4)
        oproj(0, (0, 1), True)
        oproj(1, (0, 1, 2), True)
        oproj(2, (0, 1, 2), True)
        oproj(3, (0, 2), True)
        wait_recv(5)
        for cc in (1, 2, 0, 3):
            oproj(cc, (3,), False)
        wait_recv(6)
        oproj(3, (1,), False)
        oproj(0, (2,), False)
        if comm:
            for d in cw + ccw:
                d.wait_send()

    any_spec = pl.BlockSpec(memory_space=pl.ANY)
    return pl.pallas_call(
        body,
        out_shape=jax.ShapeDtypeStruct((B_LOC, S, DM), F32),
        in_specs=[any_spec] * 5,
        out_specs=pl.BlockSpec(memory_space=pltpu.VMEM),
        scratch_shapes=[
            pltpu.VMEM((2, DM, 128), F32),
            pltpu.VMEM((GW, DM), F32),
            pltpu.VMEM((B_LOC, S, DM), F32),
            pltpu.VMEM((B_LOC, S, DM), BF),
            pltpu.VMEM((4, B_LOC, GW, S), F32),
            pltpu.VMEM((4, B_LOC, GW, S), F32),
            pltpu.VMEM((4, 2, DM, 128), BF),
            pltpu.VMEM((4, 4, GW, 128), BF),
            pltpu.VMEM((B_LOC, S, 4 * GW), BF),
            pltpu.SemaphoreType.DMA((12,)),
            pltpu.SemaphoreType.DMA((14,)),
            pltpu.SemaphoreType.DMA((14,)),
        ],
        compiler_params=pltpu.CompilerParams(
            collective_id=0 if comm else None, vmem_limit_bytes=64 * 1024 * 1024),
    )(x, Wq, Kt, Vt, Wo)


def pallas_dist_sparse_attn_causalblk_htp_bs_b2_sq256_skv256_hq4_dh64_kernel(x, Wq, K_ext, V_ext, Wo):
    return kernel(x, Wq, K_ext, V_ext, Wo)
```

```python
import jax
import jax.numpy as jnp
from jax import lax
from jax.experimental import pallas as pl
from jax.experimental.pallas import tpu as pltpu

N_DEV = 4
B_LOC = 2
S = 256
DM = 512
DH = 64
GW = 256
NEG = -1e9
LOG2E = 1.4426950408889634
QSCALE = 0.125 * LOG2E
BF = jnp.bfloat16
F32 = jnp.float32
MESH = pl.DeviceIdType.MESH

NN = (((1,), (0,)), ((), ()))
NT = (((1,), (1,)), ((), ()))


def _dot(a, b, dims=NN):
    return lax.dot_general(a, b, dims, preferred_element_type=F32)


class _NoScope:
    def __enter__(self):
        return self
    def __exit__(self, *a):
        return False


def kernel(x, Wq, K_ext, V_ext, Wo, compute=True, scopes=False, head=24,
           wq_order=((0, 24), (0, 48), (0, 128), (1, 120), (0, 288), (1, 368)), checks=False, npre=1):
    Kt = jnp.transpose(K_ext, (0, 2, 3, 1)).reshape(8, 16 * DH, S)
    Vt = jnp.transpose(V_ext, (0, 2, 3, 1)).reshape(8, 16 * DH, S)
    scope = (lambda n: jax.named_scope(n)) if scopes else (lambda n: _NoScope())
    pieces = []
    _off = [head, head]
    for j, n in wq_order:
        pieces.append((j, _off[j], n)); _off[j] += n
    assert _off == [DM, DM]
    npc = len(pieces)

    def body(x_hbm, wq_hbm, kt_hbm, vt_hbm, wo_hbm, out_ref,
             wq_f, wo_f, x_f, x_b, k_f, v_f, wq_b, wo_b, ctx, land,
             lsem, ssem, rsem, rdy):
        nl = [0]
        def lcopy(src, dst):
            i = nl[0]; nl[0] += 1
            return pltpu.make_async_copy(src, dst, lsem.at[i])

        my = lax.axis_index("i")
        c1 = (my == 1).astype(jnp.int32)
        cc = (c1, 1 - c1)
        ld_wq = [lcopy(wq_hbm.at[pl.ds(o, n), pl.ds(pl.multiple_of(cc[j] * 128, 128), 128)],
                       wq_f.at[cc[j], pl.ds(o, n)]) for j, o, n in pieces]
        for d in ld_wq[:npre]: d.start()
        right = (my + 1) % N_DEV
        left = (my + 3) % N_DEV
        odd = my % 2 == 1
        early = [my != 1, my != 3]

        def rcopy(src, dst, i, dev):
            return pltpu.make_async_remote_copy(
                src_ref=src, dst_ref=dst, send_sem=ssem.at[i], recv_sem=rsem.at[i],
                device_id=(dev,), device_id_type=MESH)

        NK = 10
        fw_rows = [(0, 256), (256, 128), (384, 64), (448, 64)]
        body_rows = pl.ds(head, DM - head)

        def link(d):
            dev = right if d == 0 else left
            sl = 1 + d
            o = d * NK
            l = [
                rcopy(wq_b.at[0, d, body_rows], wq_b.at[sl, d, body_rows], o + 0, dev),
                rcopy(wq_b.at[0, 1 - d], wq_b.at[sl, 1 - d], o + 1, dev),
                rcopy(wq_b.at[sl, d], wq_b.at[3, d], o + 2, dev),
                rcopy(wo_b.at[0, d], wo_b.at[sl, d], o + 3, dev),
                rcopy(wo_b.at[0, 1 - d], wo_b.at[sl, 1 - d], o + 4, dev),
            ]
            for p, (ro, rn) in enumerate(fw_rows):
                l.append(rcopy(wo_b.at[sl, d, pl.ds(ro, rn)], wo_b.at[3, d, pl.ds(ro, rn)], o + 5 + p, dev))
            l.append(rcopy(wq_hbm.at[pl.ds(0, head), pl.ds(d * 128, 128)], land.at[d], o + 9, dev))
            l.append(rcopy(wq_f.at[d, pl.ds(0, head)], land.at[d], o + 9, dev))
            return l

        links = [link(0), link(1)]

        bar = pltpu.get_barrier_semaphore()

        @pl.when(odd)
        def _():
            pl.semaphore_wait(bar, 1)
        @pl.when(my == 3)
        def _():
            links[0][9].start()
        @pl.when(my == 1)
        def _():
            links[1][9].start()

        @pl.when(my != 2)
        def _():
            for nb in (left, right):
                pl.semaphore_signal(bar, inc=1, device_id=(nb,), device_id_type=MESH)
        @pl.when(my == 2)
        def _():
            pl.semaphore_wait(bar, 2)
            links[0][9].start(); links[1][9].start()
            for nb in (left, right):
                pl.semaphore_signal(rdy, inc=1, device_id=(nb,), device_id_type=MESH)

        ld_wqh = [lcopy(wq_hbm.at[pl.ds(0, head), pl.ds(c * 128, 128)], wq_f.at[c, pl.ds(0, head)])
                  for c in range(2)]
        ld_x = [lcopy(x_hbm.at[b], x_f.at[b]) for b in range(B_LOC)]
        ld_wo = lcopy(wo_hbm, wo_f)
        grp = [my, left, right, (my + 2) % N_DEV]

        def kv_copy(slot, c, bs):
            rows = pl.ds(pl.multiple_of(grp[slot] * GW + c * 128, 128), 128)
            b0, nb = bs
            return [lcopy(src.at[pl.ds(B_LOC * my + b0, nb), rows, :],
                          dst.at[slot, c, pl.ds(b0, nb)])
                    for src, dst in ((kt_hbm, k_f), (vt_hbm, v_f))]

        ld_kv00 = [kv_copy(0, 0, (b, 1)) for b in range(B_LOC)]
        ld_kv = {(s, c): kv_copy(s, c, (0, 2))
                 for (s, c) in ((0, 1), (1, 0), (2, 1), (1, 1), (2, 0), (3, 0), (3, 1))}

        for d in ld_wq[npre:]: d.start()
        for d in ld_wqh: d.start()
        ld_x[0].start()
        for d in ld_kv00[0]: d.start()
        ld_x[1].start()
        for d in ld_kv00[1]: d.start()
        for key in ((0, 1), (1, 0), (2, 1)):
            for d in ld_kv[key]: d.start()
        ld_wo.start()
        for key in ((1, 1), (2, 0), (3, 0), (3, 1)):
            for d in ld_kv[key]: d.start()

        def start(k):
            links[0][k].start(); links[1][k].start()

        def wait_recv(k):
            with scope(f"recv{k}"):
                links[0][k].wait_recv(); links[1][k].wait_recv()

        with scope("bar"):
            @pl.when(my == 0)
            def _():
                pl.semaphore_wait(bar, 2)

        devs = (jnp.where(c1 == 1, left, right), jnp.where(c1 == 1, right, left))
        for i, (j, o, n) in enumerate(pieces):
            rows = pl.ds(o, n)
            c = cc[j]
            with scope(f"ldwq{i}"):
                ld_wq[i].wait()
            wq_b[0, c, rows] = wq_f[c, rows].astype(BF)
            cp = rcopy(wq_b.at[0, c, rows], wq_b.at[1 + c, c, rows], c * NK, devs[j])
            if j == 0:
                cp.start()
            else:
                pl.when(jnp.logical_not(odd))(cp.start)
        for c in range(2):
            ld_wqh[c].wait()
            wq_b[0, c, pl.ds(0, head)] = wq_f[c, pl.ds(0, head)].astype(BF)
        @pl.when(my == 0)
        def _():
            links[0][10].start(); links[1][10].start()
        for d in range(2):
            pl.when(early[d])(links[d][1].start)
        with scope("rdy"):
            for d in range(2):
                @pl.when(jnp.logical_not(early[d]))
                def _():
                    pl.semaphore_wait(rdy, 1)
                    links[d][10].start(); links[d][0].start(); links[d][1].start()

        def conv_x(b):
            with scope(f"ldx{b}"):
                ld_x[b].wait()
            for kt in range(4):
                x_b[b, kt] = x_f[b, :, pl.ds(kt * 128, 128)].astype(BF)

        lane = lax.broadcasted_iota(jnp.int32, (128, 128), 1)
        row = lax.broadcasted_iota(jnp.int32, (128, 128), 0)
        dmask = jnp.logical_and(row < 64, lane >= 64)
        lo_lane = lane < 64
        zeros_h = jnp.zeros((DH, 128), F32)
        ones_h = jnp.ones((DH, 128), F32)
        negc = NEG * LOG2E

        def stage_q(u):
            slot, c, b = u
            acc = None
            for kt in range(4):
                t = _dot(x_b[b, kt], wq_b[slot, c, pl.ds(kt * 128, 128), :])
                acc = t if acc is None else acc + t
            q = acc * QSCALE
            return q[:128].astype(BF), q[128:].astype(BF)

        def kv_tile(ref, u, hh, half, fill):
            slot, c, b = u
            t = ref[slot, c, b, pl.ds(hh * DH, DH), pl.ds(half * 128, 128)]
            parts = [t, fill] if hh == 0 else [fill, t]
            return jnp.concatenate(parts, axis=0).astype(BF)

        def stage_s(u, q):
            qt, qb = q
            res = []
            for hh in range(2):
                ka = kv_tile(k_f, u, hh, 0, zeros_h)
                kb = kv_tile(k_f, u, hh, 1, zeros_h)
                res.append((_dot(qt, ka), _dot(qb, ka), _dot(qb, kb)))
            return res

        def stage_p(s):
            res = []
            for (s_tl, s_bl, s_br) in s:
                s_tl = jnp.where(dmask, negc, s_tl)
                s_br = jnp.where(dmask, negc, s_br)
                m_t = jnp.max(s_tl, axis=1, keepdims=True)
                m_b = jnp.max(jnp.maximum(s_bl, s_br), axis=1, keepdims=True)
                res.append((jnp.exp2(s_tl - m_t).astype(BF),
                            jnp.exp2(s_bl - m_b).astype(BF),
                            jnp.exp2(s_br - m_b).astype(BF)))
            return res

        def stage_o(u, p):
            slot, c, b = u
            o = []
            for hh in range(2):
                va = kv_tile(v_f, u, hh, 0, ones_h)
                vb = kv_tile(v_f, u, hh, 1, ones_h)
                o.append((_dot(p[hh][0], va, NT),
                          _dot(p[hh][1], va, NT) + _dot(p[hh][2], vb, NT)))
            for half in range(2):
                o0, o1 = o[0][half], o[1][half]
                num = jnp.where(lo_lane, o0, o1)
                den = pltpu.roll(jnp.where(lo_lane, o1, o0), 64, 1)
                r = pl.reciprocal(den, approx=True)
                r = r * (2.0 - den * r)
                ctx[b, slot * 2 + c, pl.ds(half * 128, 128), :] = (num * r).astype(BF)

        def oproj(col, terms, init, rsplit=1):
            if not compute:
                return
            rb = S // rsplit
            cs = pl.ds(col * 128, 128)
            for b in range(B_LOC):
                for r in range(rsplit):
                    rows = pl.ds(r * rb, rb)
                    acc = None
                    for (s, pr) in terms:
                        if col < 3:
                            w = wo_b[s, pr, pl.ds(col * 128, 128), :]
                        else:
                            rr = pl.ds(384 + pr * DH, DH)
                            w = jnp.concatenate([wo_b[s, 0, rr, :], wo_b[s, 1, rr, :]], axis=0)
                        t = _dot(ctx[b, s * 2 + pr, rows], w)
                        acc = t if acc is None else acc + t
                    if init:
                        out_ref[b, rows, cs] = acc
                    else:
                        out_ref[b, rows, cs] += acc

        if not compute:
            out_ref[...] = jnp.zeros(out_ref.shape, F32)

        def wait_all(ds, name):
            with scope(name):
                for d in ds: d.wait()

        units = [(s, c, b) for (s, c) in ((0, 0), (0, 1), (1, 0), (2, 1), (1, 1), (2, 0), (3, 0), (3, 1))
                 for b in range(B_LOC)]

        def conv_wo():
            with scope("ldwo"):
                ld_wo.wait()
            for h in range(2):
                for col in range(3):
                    wo_b[0, h, pl.ds(col * 128, 128), :] = wo_f[pl.ds(h * 128, 128),
                                                                pl.ds(col * 128, 128)].astype(BF)
                for pr in range(2):
                    wo_b[0, h, pl.ds(384 + pr * DH, DH), :] = wo_f[pl.ds(pr * 128 + h * DH, DH),
                                                                   pl.ds(384, 128)].astype(BF)

        def pre(i):
            if i == 0:
                conv_x(0); wait_all(ld_kv00[0], "ldkv00a")
            elif i == 1:
                conv_x(1); wait_all(ld_kv00[1], "ldkv00b")
            elif i == 2:
                wait_all(ld_kv[0, 1], "ldkv01")
            elif i == 4:
                wait_recv(9); wait_recv(0)
                for d in range(2):
                    wq_b[1 + d, d, pl.ds(0, head)] = land[d].astype(BF)
                start(2)
                conv_wo()
                start(3); start(4)
                wait_all(ld_kv[1, 0] + ld_kv[2, 1], "ldkvA")
            elif i == 8:
                wait_recv(1); wait_all(ld_kv[1, 1] + ld_kv[2, 0], "ldkvB")
            elif i == 12:
                wait_recv(2); wait_all(ld_kv[3, 0] + ld_kv[3, 1], "ldkvD")

        if not compute:
            for i in range(len(units)): pre(i)
        else:
            pend = None
            for i, u in enumerate(units):
                pre(i)
                s = stage_s(u, stage_q(u))
                if pend is not None:
                    stage_o(*pend)
                pend = (u, stage_p(s))
            stage_o(*pend)

        wait_recv(3)
        for p in range(4):
            start(5 + p)
        for col in range(3):
            oproj(col, [(0, 0), (0, 1), (1, 0), (2, 1)], True)
        oproj(3, [(0, 0), (0, 1)], True)
        wait_recv(4)
        oproj(3, [(1, 0), (1, 1), (2, 0), (2, 1)], False)
        for col in range(3):
            oproj(col, [(1, 1), (2, 0)], False)
        with scope("sendw"):
            for l in links:
                for d in l[:5] + l[9:10]:
                    d.wait_send()
        wait_recv(5)
        oproj(0, [(3, 0), (3, 1)], False)
        oproj(1, [(3, 0), (3, 1)], False)
        wait_recv(6)
        oproj(2, [(3, 0), (3, 1)], False)
        wait_recv(7)
        oproj(3, [(3, 0)], False, 2)
        for l in links:
            for d in l[5:9]:
                d.wait_send()
        wait_recv(8)
        oproj(3, [(3, 1)], False, 2)

    any_spec = pl.BlockSpec(memory_space=pl.ANY)
    return pl.pallas_call(
        body,
        out_shape=jax.ShapeDtypeStruct((B_LOC, S, DM), F32),
        in_specs=[any_spec] * 5,
        out_specs=pl.BlockSpec(memory_space=pltpu.VMEM),
        scratch_shapes=[
            pltpu.VMEM((2, DM, 128), F32),
            pltpu.VMEM((GW, DM), F32),
            pltpu.VMEM((B_LOC, S, DM), F32),
            pltpu.VMEM((B_LOC, 4, S, 128), BF),
            pltpu.VMEM((4, 2, B_LOC, 128, S), F32),
            pltpu.VMEM((4, 2, B_LOC, 128, S), F32),
            pltpu.VMEM((4, 2, DM, 128), BF),
            pltpu.VMEM((4, 2, DM, 128), BF),
            pltpu.VMEM((B_LOC, 8, S, 128), BF),
            pltpu.VMEM((2, head, 128), F32),
            pltpu.SemaphoreType.DMA((npc + 23,)),
            pltpu.SemaphoreType.DMA((20,)),
            pltpu.SemaphoreType.DMA((20,)),
            pltpu.SemaphoreType.REGULAR,
        ],
        compiler_params=pltpu.CompilerParams(
            collective_id=0, vmem_limit_bytes=64 * 1024 * 1024,
            disable_bounds_checks=not checks, disable_semaphore_checks=not checks),
    )(x, Wq, Kt, Vt, Wo)


def pallas_dist_sparse_attn_causalblk_htp_bs_b2_sq256_skv256_hq4_dh64_kernel(x, Wq, K_ext, V_ext, Wo):
    return kernel(x, Wq, K_ext, V_ext, Wo)
```

```python
import jax
import jax.numpy as jnp
from jax import lax
from jax.experimental import pallas as pl
from jax.experimental.pallas import tpu as pltpu

B_LOC = 2
S = 256
DM = 512
DH = 64
GW = 256
LOG2E = 1.4426950408889634
QSCALE = 0.125 * LOG2E
NEG = -1e9 * LOG2E
BF = jnp.bfloat16
F32 = jnp.float32
MESH = pl.DeviceIdType.MESH

NN = (((1,), (0,)), ((), ()))
NT = (((1,), (1,)), ((), ()))

NK = 10
HEAD = 24
WQ_PIECES = ((0, 0, 16), (0, 16, 32), (0, 48, 64), (0, 112, 128), (1, 0, 128),
             (0, 240, 272), (1, 128, 384))
FW_ROWS = ((0, 256), (256, 128), (384, 64), (448, 64))
PAIRS = ((0, 0), (0, 1), (1, 0), (2, 1), (1, 1), (2, 0), (3, 0), (3, 1))


def _dot(a, b, dims=NN):
    return lax.dot_general(a, b, dims, preferred_element_type=F32)


def _body(x_hbm, wq_hbm, kt_hbm, vt_hbm, wo_hbm, out_ref,
          wq_f, wo_f, x_f, x_b, k_f, v_f, wq_b, wo_b, ctx, land,
          lsem, ssem, rsem, rdy):
    n_local = [0]

    def lcopy(src, dst):
        n_local[0] += 1
        return pltpu.make_async_copy(src, dst, lsem.at[n_local[0] - 1])

    def rcopy(src, dst, i, dev):
        return pltpu.make_async_remote_copy(
            src_ref=src, dst_ref=dst, send_sem=ssem.at[i], recv_sem=rsem.at[i],
            device_id=(dev,), device_id_type=MESH)

    def lanes(c):
        return pl.ds(pl.multiple_of(c * 128, 128), 128)

    my = lax.axis_index("i")
    odd = (my & 1) == 1
    c1 = (my == 1).astype(jnp.int32)
    cc = (c1, 1 - c1)
    head_rows = pl.ds(DM - HEAD, HEAD)
    body_rows = pl.ds(0, DM - HEAD)

    ld_wq = [lcopy(wq_hbm.at[pl.ds(o, n), lanes(cc[j])], wq_f.at[cc[j], pl.ds(o, n)])
             for j, o, n in WQ_PIECES]
    ld_wq[0].start()

    bar = pltpu.get_barrier_semaphore()

    @pl.when(odd)
    def _():
        pl.semaphore_wait(bar, 1)
        rcopy(wq_hbm.at[head_rows, lanes(c1)], land.at[c1], c1 * NK + 9, 0).start()

    right = (my + 1) & 3
    left = (my + 3) & 3

    @pl.when(my != 2)
    def _():
        for nb in (left, right):
            pl.semaphore_signal(bar, inc=1, device_id=(nb,), device_id_type=MESH)

    @pl.when(my == 2)
    def _():
        pl.semaphore_wait(bar, 2)
        for d, nb in enumerate((3, 1)):
            rcopy(wq_hbm.at[head_rows, pl.ds(d * 128, 128)], land.at[d], d * NK + 9, nb).start()
        for nb in (1, 3):
            pl.semaphore_signal(rdy, inc=1, device_id=(nb,), device_id_type=MESH)

    def link(d):
        dev = (right, left)[d]
        sl, o = 1 + d, d * NK
        return [
            rcopy(wq_b.at[0, d, body_rows], wq_b.at[sl, d, body_rows], o + 0, dev),
            rcopy(wq_b.at[0, 1 - d], wq_b.at[sl, 1 - d], o + 1, dev),
            rcopy(wq_b.at[sl, d], wq_b.at[3, d], o + 2, dev),
            rcopy(wo_b.at[0, d], wo_b.at[sl, d], o + 3, dev),
            rcopy(wo_b.at[0, 1 - d], wo_b.at[sl, 1 - d], o + 4, dev),
        ] + [
            rcopy(wo_b.at[sl, d, pl.ds(ro, rn)], wo_b.at[3, d, pl.ds(ro, rn)], o + 5 + p, dev)
            for p, (ro, rn) in enumerate(FW_ROWS)
        ] + [
            rcopy(wq_f.at[d, head_rows], land.at[d], o + 9, dev),
        ]

    links = [link(0), link(1)]

    def start(k):
        links[0][k].start()
        links[1][k].start()

    def wait_recv(k):
        links[0][k].wait_recv()
        links[1][k].wait_recv()

    def wait_send(ks):
        for l in links:
            for k in ks:
                l[k].wait_send()

    def wait_all(ds):
        for d in ds:
            d.wait()

    grp = (my, left, right, (my + 2) & 3)

    def kv_copy(slot, c, b0, nb):
        rows = pl.ds(pl.multiple_of(grp[slot] * GW + c * 128, 128), 128)
        return [lcopy(src.at[pl.ds(B_LOC * my + b0, nb), rows, :], dst.at[slot, c, pl.ds(b0, nb)])
                for src, dst in ((kt_hbm, k_f), (vt_hbm, v_f))]

    ld_x = [lcopy(x_hbm.at[b], x_f.at[b]) for b in range(B_LOC)]
    ld_wo = lcopy(wo_hbm, wo_f)
    ld_kv0 = [kv_copy(0, 0, b, 1) for b in range(B_LOC)]
    ld_kv = [None] + [kv_copy(s, c, 0, B_LOC) for s, c in PAIRS[1:]]
    for d in (ld_wq[1:] + [ld_x[0]] + ld_kv0[0] + [ld_x[1]] + ld_kv0[1]
              + ld_kv[1] + ld_kv[2] + ld_kv[3] + [ld_wo]
              + ld_kv[4] + ld_kv[5] + ld_kv[6] + ld_kv[7]):
        d.start()

    @pl.when(my == 0)
    def _():
        pl.semaphore_wait(bar, 2)

    devs = (jnp.where(c1 == 1, left, right), jnp.where(c1 == 1, right, left))
    for i, (j, o, n) in enumerate(WQ_PIECES):
        c = cc[j]
        ld_wq[i].wait()
        wq_b[0, c, pl.ds(o, n)] = wq_f[c, pl.ds(o, n)].astype(BF)
        rows = pl.ds(o, min(n, DM - HEAD - o))
        cp = rcopy(wq_b.at[0, c, rows], wq_b.at[1 + c, c, rows], c * NK, devs[j])
        if j == 0:
            cp.start()
        else:
            pl.when(jnp.logical_not(odd))(cp.start)

    @pl.when(my == 0)
    def _():
        start(9)

    for d, late in enumerate((1, 3)):
        pl.when(my != late)(links[d][1].start)
    for d, late in enumerate((1, 3)):
        @pl.when(my == late)
        def _():
            pl.semaphore_wait(rdy, 1)
            for k in (9, 0, 1):
                links[d][k].start()

    lane = lax.broadcasted_iota(jnp.int32, (128, 128), 1)
    row = lax.broadcasted_iota(jnp.int32, (128, 128), 0)
    dmask = jnp.logical_and(row < 64, lane >= 64)
    lo_lane = lane < 64
    zeros_h = jnp.zeros((DH, 128), F32)
    ones_h = jnp.ones((DH, 128), F32)

    def stage_q(u):
        slot, c, b = u
        acc = None
        for kt in range(4):
            t = _dot(x_b[b, kt], wq_b[slot, c, pl.ds(kt * 128, 128), :])
            acc = t if acc is None else acc + t
        q = acc * QSCALE
        return q[:128].astype(BF), q[128:].astype(BF)

    def kv_tile(ref, u, hh, half, fill):
        slot, c, b = u
        t = ref[slot, c, b, pl.ds(hh * DH, DH), pl.ds(half * 128, 128)]
        return jnp.concatenate([t, fill] if hh == 0 else [fill, t], axis=0).astype(BF)

    def stage_s(u, q):
        qt, qb = q
        res = []
        for hh in range(2):
            ka = kv_tile(k_f, u, hh, 0, zeros_h)
            kb = kv_tile(k_f, u, hh, 1, zeros_h)
            res.append((_dot(qt, ka), _dot(qb, ka), _dot(qb, kb)))
        return res

    def stage_p(s):
        res = []
        for s_tl, s_bl, s_br in s:
            s_tl = jnp.where(dmask, NEG, s_tl)
            s_br = jnp.where(dmask, NEG, s_br)
            m_t = jnp.max(s_tl, axis=1, keepdims=True)
            m_b = jnp.max(jnp.maximum(s_bl, s_br), axis=1, keepdims=True)
            res.append((jnp.exp2(s_tl - m_t).astype(BF),
                        jnp.exp2(s_bl - m_b).astype(BF),
                        jnp.exp2(s_br - m_b).astype(BF)))
        return res

    def stage_o(u, p):
        slot, c, b = u
        o = []
        for hh in range(2):
            va = kv_tile(v_f, u, hh, 0, ones_h)
            vb = kv_tile(v_f, u, hh, 1, ones_h)
            o.append((_dot(p[hh][0], va, NT),
                      _dot(p[hh][1], va, NT) + _dot(p[hh][2], vb, NT)))
        for half in range(2):
            o0, o1 = o[0][half], o[1][half]
            num = jnp.where(lo_lane, o0, o1)
            den = pltpu.roll(jnp.where(lo_lane, o1, o0), 64, 1)
            ctx[b, slot * 2 + c, pl.ds(half * 128, 128), :] = (num / den).astype(BF)

    def conv_x(b):
        ld_x[b].wait()
        for kt in range(4):
            x_b[b, kt] = x_f[b, :, pl.ds(kt * 128, 128)].astype(BF)

    def conv_wo():
        ld_wo.wait()
        for h in range(2):
            for col in range(3):
                wo_b[0, h, pl.ds(col * 128, 128), :] = (
                    wo_f[pl.ds(h * 128, 128), pl.ds(col * 128, 128)].astype(BF))
            for pr in range(2):
                wo_b[0, h, pl.ds(384 + pr * DH, DH), :] = (
                    wo_f[pl.ds(pr * 128 + h * DH, DH), pl.ds(384, 128)].astype(BF))

    def before_unit(i):
        if i < 2:
            conv_x(i)
            wait_all(ld_kv0[i])
        elif i == 2:
            wait_all(ld_kv[1])
        elif i == 4:
            wait_recv(9)
            wait_recv(0)
            for d in range(2):
                wq_b[1 + d, d, head_rows] = land[d].astype(BF)
            start(2)
            conv_wo()
            start(3)
            start(4)
            wait_all(ld_kv[2] + ld_kv[3])
        elif i == 8:
            wait_recv(1)
            wait_all(ld_kv[4] + ld_kv[5])
        elif i == 12:
            wait_recv(2)
            wait_all(ld_kv[6] + ld_kv[7])

    pending = None
    for i, u in enumerate((s, c, b) for s, c in PAIRS for b in range(B_LOC)):
        before_unit(i)
        s = stage_s(u, stage_q(u))
        if pending is not None:
            stage_o(*pending)
        pending = (u, stage_p(s))
    stage_o(*pending)

    def oproj(col, terms, init=False, rsplit=1):
        rb = S // rsplit
        cs = pl.ds(col * 128, 128)
        for b in range(B_LOC):
            for r in range(rsplit):
                rows = pl.ds(r * rb, rb)
                acc = None
                for s, pr in terms:
                    if col < 3:
                        w = wo_b[s, pr, pl.ds(col * 128, 128), :]
                    else:
                        rr = pl.ds(384 + pr * DH, DH)
                        w = jnp.concatenate([wo_b[s, 0, rr, :], wo_b[s, 1, rr, :]], axis=0)
                    t = _dot(ctx[b, s * 2 + pr, rows], w)
                    acc = t if acc is None else acc + t
                if init:
                    out_ref[b, rows, cs] = acc
                else:
                    out_ref[b, rows, cs] += acc

    wait_recv(3)
    for p in range(len(FW_ROWS)):
        start(5 + p)
    for col in range(3):
        oproj(col, [(0, 0), (0, 1), (1, 0), (2, 1)], init=True)
    oproj(3, [(0, 0), (0, 1)], init=True)
    wait_recv(4)
    oproj(3, [(1, 0), (1, 1), (2, 0), (2, 1)])
    for col in range(3):
        oproj(col, [(1, 1), (2, 0)])
    wait_send((0, 1, 2, 3, 4, 9))
    wait_recv(5)
    oproj(0, [(3, 0), (3, 1)])
    oproj(1, [(3, 0), (3, 1)])
    wait_recv(6)
    oproj(2, [(3, 0), (3, 1)])
    wait_recv(7)
    oproj(3, [(3, 0)], rsplit=2)
    wait_send((5, 6, 7))
    wait_recv(8)
    oproj(3, [(3, 1)], rsplit=2)
    wait_send((8,))


def pallas_dist_sparse_attn_causalblk_htp_bs_b2_sq256_skv256_hq4_dh64_kernel(
    x: jax.Array,
    Wq: jax.Array,
    K_ext: jax.Array,
    V_ext: jax.Array,
    Wo: jax.Array,
):
    Kt = jnp.transpose(K_ext, (0, 2, 3, 1)).reshape(8, 16 * DH, S)
    Vt = jnp.transpose(V_ext, (0, 2, 3, 1)).reshape(8, 16 * DH, S)
    return pl.pallas_call(
        _body,
        out_shape=jax.ShapeDtypeStruct((B_LOC, S, DM), F32),
        in_specs=[pl.BlockSpec(memory_space=pl.ANY)] * 5,
        out_specs=pl.BlockSpec(memory_space=pltpu.VMEM),
        scratch_shapes=[
            pltpu.VMEM((2, DM, 128), F32),
            pltpu.VMEM((GW, DM), F32),
            pltpu.VMEM((B_LOC, S, DM), F32),
            pltpu.VMEM((B_LOC, 4, S, 128), BF),
            pltpu.VMEM((4, 2, B_LOC, 128, S), F32),
            pltpu.VMEM((4, 2, B_LOC, 128, S), F32),
            pltpu.VMEM((4, 2, DM, 128), BF),
            pltpu.VMEM((4, 2, DM, 128), BF),
            pltpu.VMEM((B_LOC, 8, S, 128), BF),
            pltpu.VMEM((2, HEAD, 128), F32),
            pltpu.SemaphoreType.DMA((len(WQ_PIECES) + 21,)),
            pltpu.SemaphoreType.DMA((2 * NK,)),
            pltpu.SemaphoreType.DMA((2 * NK,)),
            pltpu.SemaphoreType.REGULAR,
        ],
        compiler_params=pltpu.CompilerParams(
            collective_id=0, vmem_limit_bytes=32 * 1024 * 1024,
            disable_bounds_checks=True, disable_semaphore_checks=True),
    )(x, Wq, Kt, Vt, Wo)
```
